```python
import numpy as np

kernel_name = "dist_mean_ax0_shard0_i_m4096_n1024"

def setup_inputs():
    return {"x": np.random.randn(16384, 1024).astype(np.float32)}

def reference(x: np.ndarray) -> np.ndarray:
    return np.mean(x, axis=0, keepdims=True)
```

```python
import jax
import jax.numpy as jnp
from jax import lax
from jax.experimental import pallas as pl
from jax.experimental.pallas import tpu as pltpu

N_DEV = 4
MESH = pl.DeviceIdType.MESH
UNROLL = 8

CHUNKS = (416, 36, 4)
LENT = 28


def _sum_groups(ref, start, count, acc):
    loops = count // UNROLL if count >= 2 * UNROLL else 0
    if loops:

        def step(i, a):
            for u in range(UNROLL):
                a = a + ref[start + i * UNROLL + u]
            return a

        acc = lax.fori_loop(0, loops, step, acc)
    for g in range(loops * UNROLL, count):
        acc = acc + ref[start + g]
    return acc


def _fold(acc):
    tiles = [acc[:, 128 * j : 128 * (j + 1)] for j in range(8)]
    sublane = lax.broadcasted_iota(jnp.int32, (8, 128), 0)
    for k in (4, 2, 1):
        upper = (sublane & k) != 0
        half = len(tiles) // 2
        folded = []
        for a, b in zip(tiles[:half], tiles[half:]):
            moved = jnp.where(upper, pltpu.roll(b, k, 0), pltpu.roll(a, 8 - k, 0))
            folded.append(jnp.where(upper, b, a) + moved)
        tiles = folded
    return tiles[0]


def pallas_dist_mean_ax0_shard0_i_m4096_n1024_kernel(
    x: jax.Array,
):
    m, n = x.shape
    groups = m // 8
    local = sum(CHUNKS)
    starts = [sum(CHUNKS[:c]) for c in range(len(CHUNKS))]
    assert n == 1024 and local + 2 * LENT == groups

    def body(x_ref, o_ref, buf, inbox, mine, got, load_sem, lend_send, lend_recv, send_sem, recv_sem):
        loads = [
            pltpu.make_async_copy(x_ref.at[pl.ds(s, c)], buf.at[pl.ds(s, c)], load_sem.at[i])
            for i, (s, c) in enumerate(zip(starts, CHUNKS))
        ]
        for load in loads:
            load.start()

        me = lax.axis_index("i")
        diagonal, right, left = ((me + d) & (N_DEV - 1) for d in (2, 1, 3))
        barrier = pltpu.get_barrier_semaphore()
        for peer in (diagonal, right, left):
            pl.semaphore_signal(barrier, inc=1, device_id=(peer,), device_id_type=MESH)
        pl.semaphore_wait(barrier, N_DEV - 1)

        lends = [
            pltpu.make_async_remote_copy(
                x_ref.at[pl.ds(local + j * LENT, LENT)],
                inbox.at[j],
                lend_send.at[j],
                lend_recv.at[j],
                device_id=(peer,),
                device_id_type=MESH,
            )
            for j, peer in enumerate((right, left))
        ]
        for lend in lends:
            lend.start()

        acc = jnp.zeros((8, n), jnp.float32)
        for i, load in enumerate(loads):
            if i == 1:
                for j, lend in enumerate(lends):
                    lend.wait_recv()
                    acc = _sum_groups(inbox.at[j], 0, LENT, acc)
            load.wait()
            acc = _sum_groups(buf, starts[i], CHUNKS[i], acc)

        part = _fold(acc) * (1.0 / (N_DEV * m))
        mine[...] = part
        sends = [
            pltpu.make_async_remote_copy(
                mine, got.at[k], send_sem.at[k], recv_sem.at[k], device_id=(peer,), device_id_type=MESH
            )
            for k, peer in enumerate((diagonal, right, left))
        ]
        for send in sends:
            send.start()
        for copy in lends + sends:
            copy.wait_send()
        sends[1].wait_recv()
        sends[2].wait_recv()
        total = part + got[1] + got[2]
        sends[0].wait_recv()
        o_ref[...] = total + got[0]

    out = pl.pallas_call(
        body,
        out_shape=jax.ShapeDtypeStruct((8, 128), jnp.float32),
        in_specs=[pl.BlockSpec(memory_space=pl.ANY)],
        out_specs=pl.BlockSpec(memory_space=pltpu.VMEM),
        scratch_shapes=[
            pltpu.VMEM((local, 8, n), jnp.float32),
            pltpu.VMEM((2, LENT, 8, n), jnp.float32),
            pltpu.VMEM((8, 128), jnp.float32),
            pltpu.VMEM((N_DEV - 1, 8, 128), jnp.float32),
            pltpu.SemaphoreType.DMA((len(CHUNKS),)),
            pltpu.SemaphoreType.DMA((2,)),
            pltpu.SemaphoreType.DMA((2,)),
            pltpu.SemaphoreType.DMA((N_DEV - 1,)),
            pltpu.SemaphoreType.DMA((N_DEV - 1,)),
        ],
        compiler_params=pltpu.CompilerParams(
            collective_id=0,
            vmem_limit_bytes=48 * 1024 * 1024,
            disable_bounds_checks=True,
            disable_semaphore_checks=True,
        ),
    )(x.reshape(groups, 8, n))
    return out.reshape(1, n)
```

```python
import functools

import jax
import jax.numpy as jnp
from jax import lax
from jax.experimental import pallas as pl
from jax.experimental.pallas import tpu as pltpu

N_DEV = 4
SUBLANES = 8
LANES = 128
UNROLL = 16

LENT = 27
STAGED = 14
LAST = 48


def _accumulate(acc, ref):
    count = ref.shape[0]

    def step(i, a):
        for u in range(UNROLL):
            a = a + ref[i * UNROLL + u]
        return a

    acc = lax.fori_loop(0, count // UNROLL, step, acc)
    for g in range(count - count % UNROLL, count):
        acc = acc + ref[g]
    return acc


def _tree_sum(terms):
    while len(terms) > 1:
        terms = [a + b for a, b in zip(terms[::2], terms[1::2])] + terms[len(terms) // 2 * 2 :]
    return terms[0]


def _column_sums(tiles):
    row = lax.broadcasted_iota(jnp.int32, (SUBLANES, LANES), 0)
    for k in (4, 2, 1):
        upper = (row & k) != 0
        half = len(tiles) // 2
        tiles = [
            jnp.where(upper, b, a)
            + jnp.where(upper, pltpu.roll(b, k, 0), pltpu.roll(a, SUBLANES - k, 0))
            for a, b in zip(tiles[:half], tiles[half:])
        ]
    return tiles[0]


def _kernel(
    x_ref,
    out_ref,
    rows,
    inbox,
    wide,
    narrow,
    staging,
    early,
    late,
    whole,
    early_in,
    late_in,
    whole_in,
    load_sem,
    send_sem,
    recv_sem,
    *,
    total_rows,
):
    main = rows.shape[0] - STAGED
    last = pl.ds(main, LAST)
    lent_start = main + LAST
    staged_start = lent_start + 2 * LENT

    load_main = pltpu.make_async_copy(
        x_ref.at[pl.ds(0, main)], rows.at[pl.ds(0, main)], load_sem.at[0]
    )
    load_wide = pltpu.make_async_copy(
        x_ref.at[last, :, pl.ds(LANES, wide.shape[2])], wide, load_sem.at[1]
    )
    load_narrow = pltpu.make_async_copy(
        x_ref.at[last, :, pl.ds(0, LANES)], narrow, load_sem.at[2]
    )
    stage_in = pltpu.make_async_copy(
        x_ref.at[pl.ds(staged_start, STAGED)], staging, load_sem.at[3]
    )
    stage_out = pltpu.make_async_copy(
        staging, rows.at[pl.ds(main, STAGED)], load_sem.at[4]
    )
    load_main.start()
    me = lax.axis_index("i")
    diagonal, right, left = ((me + d) & (N_DEV - 1) for d in (2, 1, 3))
    load_wide.start()
    load_narrow.start()
    stage_in.start()

    barrier = pltpu.get_barrier_semaphore()
    for peer in (diagonal, right, left):
        pl.semaphore_signal(
            barrier, inc=1, device_id=(peer,), device_id_type=pl.DeviceIdType.MESH
        )
    pl.semaphore_wait(barrier, N_DEV - 1)

    def remote(i, src, dst, peer):
        return pltpu.make_async_remote_copy(
            src,
            dst,
            send_sem.at[i],
            recv_sem.at[i],
            device_id=(peer,),
            device_id_type=pl.DeviceIdType.MESH,
        )

    lends = [
        remote(
            i,
            x_ref.at[pl.ds(lent_start + i * LENT, LENT)],
            inbox.at[pl.ds(i * LENT, LENT)],
            peer,
        )
        for i, peer in enumerate((right, left))
    ]
    send_early = remote(2, early, early_in, diagonal)
    send_late = remote(3, late, late_in, diagonal)
    send_whole = [
        remote(4 + i, whole, whole_in.at[i], peer) for i, peer in enumerate((right, left))
    ]
    for lend in lends:
        lend.start()

    stage_in.wait()
    stage_out.start()
    stage_out.wait()
    load_main.wait()
    acc = _accumulate(jnp.zeros(rows.shape[1:], jnp.float32), rows)
    for lend in lends:
        lend.wait_recv()
    acc = _accumulate(acc, inbox)

    load_wide.wait()
    acc_wide = _accumulate(acc[:, LANES:], wide)
    sums_wide = _column_sums(
        [jnp.zeros((SUBLANES, LANES), jnp.float32)]
        + [acc_wide[:, c : c + LANES] for c in range(0, wide.shape[2], LANES)]
    )
    early[...] = sums_wide
    send_early.start()

    load_narrow.wait()
    sums_narrow = _tree_sum([acc[:, :LANES]] + [narrow[g] for g in range(LAST)])
    for k in (4, 2, 1):
        sums_narrow = sums_narrow + pltpu.roll(sums_narrow, k, 0)
    late[...] = sums_narrow[:1]
    send_late.start()

    row = lax.broadcasted_iota(jnp.int32, (SUBLANES, LANES), 0)
    sums = jnp.where(row == 0, sums_narrow, sums_wide)
    whole[...] = sums
    for send in send_whole:
        send.start()

    for copy in (*lends, send_early, send_late, *send_whole):
        copy.wait_send()
    for send in send_whole:
        send.wait_recv()
    send_early.wait_recv()
    total = sums + whole_in[0] + whole_in[1] + early_in[...]
    out_ref[...] = total * (1.0 / total_rows)
    send_late.wait_recv()
    out_ref[:1, :] = (total[:1] + late_in[...]) * (1.0 / total_rows)


def pallas_dist_mean_ax0_shard0_i_m4096_n1024_kernel(
    x: jax.Array,
):
    m, n = x.shape
    assert n == SUBLANES * LANES and m % SUBLANES == 0
    groups = m // SUBLANES
    main = groups - LAST - 2 * LENT - STAGED

    def vmem(*shape):
        return pltpu.VMEM(shape, jnp.float32)

    out = pl.pallas_call(
        functools.partial(_kernel, total_rows=N_DEV * m),
        out_shape=jax.ShapeDtypeStruct((SUBLANES, LANES), jnp.float32),
        in_specs=[pl.BlockSpec(memory_space=pl.ANY)],
        out_specs=pl.BlockSpec(memory_space=pltpu.VMEM),
        scratch_shapes=[
            vmem(main + STAGED, SUBLANES, n),
            vmem(2 * LENT, SUBLANES, n),
            vmem(LAST, SUBLANES, n - LANES),
            vmem(LAST, SUBLANES, LANES),
            pltpu.SMEM((STAGED, SUBLANES, n), jnp.float32),
            vmem(SUBLANES, LANES),
            vmem(1, LANES),
            vmem(SUBLANES, LANES),
            vmem(SUBLANES, LANES),
            vmem(1, LANES),
            vmem(2, SUBLANES, LANES),
            pltpu.SemaphoreType.DMA((5,)),
            pltpu.SemaphoreType.DMA((6,)),
            pltpu.SemaphoreType.DMA((6,)),
        ],
        compiler_params=pltpu.CompilerParams(
            collective_id=0,
            vmem_limit_bytes=32 * 1024 * 1024,
            disable_semaphore_checks=True,
        ),
    )(x.reshape(groups, SUBLANES, n))
    return out.reshape(1, n)
```
